```python
import numpy as np

kernel_name = "dist_sparse_attn_strided_htp_bs_b2_sq256_skv256_hq4_dh64"

def setup_inputs():
    x = np.random.randn(8, 256, 512).astype(np.float32)
    Wq = np.random.randn(512, 1024).astype(np.float32) * 0.02
    K_ext = np.random.randn(8, 256, 16, 64).astype(np.float32)
    V_ext = np.random.randn(8, 256, 16, 64).astype(np.float32)
    Wo = np.random.randn(1024, 512).astype(np.float32) * 0.02
    return {"x": x, "Wq": Wq, "K_ext": K_ext, "V_ext": V_ext, "Wo": Wo}

def reference(x, Wq, K_ext, V_ext, Wo):
    B, Sq, Skv, Hq, Dh = 8, 256, 256, 16, 64
    Q = (x @ Wq).reshape(B, Sq, Hq, Dh)
    qb = (np.arange(Sq) // 64)[:, None]
    kb = (np.arange(Skv) // 64)[None, :]
    mask = (qb == kb) | ((kb % 4) == (qb % 4))
    scores = np.einsum('bihd,bjhd->bhij', Q, K_ext).astype(np.float32) * 0.125
    scores = np.where(mask[None, None, :, :], scores, -1e9)
    scores_max = scores.max(axis=-1, keepdims=True)
    w = np.exp(scores - scores_max)
    row_keep = mask.any(axis=1)
    w_sum = np.where(row_keep[None, None, :, None], w.sum(axis=-1, keepdims=True), 1.0)
    w = w / w_sum
    w = np.where(row_keep[None, None, :, None], w, 0.0)
    ctx = np.einsum('bhij,bjhd->bihd', w, V_ext).reshape(B, Sq, Hq * Dh)
    return ctx @ Wo
```

```python
import contextlib
import jax
import jax.numpy as jnp
from jax import lax
from jax.experimental import pallas as pl
from jax.experimental.pallas import tpu as pltpu

N_DEV = 4
T = 512
D = 512
BF = jnp.bfloat16
F32 = jnp.float32
SCOPES = False
OUT_DTYPE = jnp.float32
CHECKS = False

WQ_CHUNKS = ((0, 32), (32, 96), (128, 128), (256, 256))


def scope(name):
    return jax.named_scope(name) if SCOPES else contextlib.nullcontext()


def pallas_dist_sparse_attn_strided_htp_bs_b2_sq256_skv256_hq4_dh64_kernel(x, Wq, K_ext, V_ext, Wo):
    x2 = x.reshape(T, D)
    KT = jnp.transpose(K_ext, (0, 2, 3, 1)).reshape(8, 8, 128, 256)
    VT = jnp.transpose(V_ext, (0, 2, 3, 1)).reshape(8, 8, 128, 256)

    def body(x_hbm, wq_hbm, kt_hbm, vt_hbm, wo_hbm, out_ref,
             x_f, wq_f, wo_f, kt_f, vt_f,
             x_b, wq_all, wo_all, ctx, acc,
             lsem, ssem, rsem, rdy):
        me = lax.axis_index("i")
        right = lax.rem(me + 1, N_DEV)
        left = lax.rem(me + 3, N_DEV)
        diag = lax.rem(me + 2, N_DEV)
        MESH = pl.DeviceIdType.MESH
        nbr = (right, left)

        nl = [0]

        def load(src, dst):
            cp = pltpu.make_async_copy(src, dst, lsem.at[nl[0]])
            nl[0] += 1
            cp.start()
            return cp

        wq_ld = [load(wq_hbm.at[pl.ds(o, n)], wq_f.at[pl.ds(o, n)]) for o, n in WQ_CHUNKS]

        bs = pltpu.get_barrier_semaphore()

        @pl.when(me != 2)
        def _():
            for n in nbr:
                pl.semaphore_signal(bs, inc=1, device_id=(n,), device_id_type=MESH)

        @pl.when(me == 2)
        def _():
            pl.semaphore_wait(bs, 2)
            for n in nbr:
                pl.semaphore_signal(rdy, inc=1, device_id=(n,), device_id_type=MESH)

        x_ld = load(x_hbm, x_f)
        slot_group = (me, left, right, diag)

        def load_kv(s, q):
            gp = slot_group[s] * 2 + q
            k = load(kt_hbm.at[pl.ds(2 * me, 2), gp], kt_f.at[s, q])
            v = load(vt_hbm.at[pl.ds(2 * me, 2), gp], vt_f.at[s, q])
            return k, v

        kv_ld = {}
        kv_ld[(0, 0)] = load_kv(0, 0)
        wo_ld = load(wo_hbm, wo_f)
        for sq in ((0, 1), (1, 0), (2, 1), (1, 1), (2, 0), (3, 0), (3, 1)):
            kv_ld[sq] = load_kv(*sq)

        nr = [0]
        sends = []

        def rdesc(src, dst, d):
            i = nr[0]
            nr[0] += 1
            cp = pltpu.make_async_remote_copy(src, dst, ssem.at[i], rsem.at[i],
                                              device_id=(nbr[d],), device_id_type=MESH)
            sends.append(cp)
            return cp

        def rcopy(src, dst, d):
            cp = rdesc(src, dst, d)
            cp.start()
            return cp

        a1 = [[rdesc(wq_all.at[0, d, pl.ds(o, n)], wq_all.at[1 + d, d, pl.ds(o, n)], d)
               for (o, n) in WQ_CHUNKS] for d in range(2)]
        a2 = [rdesc(wq_all.at[0, 1 - d], wq_all.at[1 + d, 1 - d], d) for d in range(2)]
        early = (me != 1, me != 3)

        for ci, (o, n) in enumerate(WQ_CHUNKS):
            with scope(f"wq_ld{ci}"):
                wq_ld[ci].wait()
            w = wq_f[pl.ds(o, n), :].astype(BF)
            wq_all[0, 0, pl.ds(o, n), :] = w[:, :128]
            wq_all[0, 1, pl.ds(o, n), :] = w[:, 128:]
            if ci == 0:
                with scope("barrier"):
                    @pl.when(me == 0)
                    def _():
                        pl.semaphore_wait(bs, 2)

                    @pl.when(lax.rem(me, 2) == 1)
                    def _():
                        pl.semaphore_wait(bs, 1)
            for d in range(2):
                @pl.when(early[d])
                def _():
                    a1[d][ci].start()
                    if ci == len(WQ_CHUNKS) - 1:
                        a2[d].start()
        with scope("rdy"):
            for d in range(2):
                @pl.when(jnp.logical_not(early[d]))
                def _():
                    pl.semaphore_wait(rdy, 1)
                    for cp in a1[d]:
                        cp.start()
                    a2[d].start()

        with scope("x_ld"):
            x_ld.wait()
        with scope("x_cast"):
            x_b[...] = x_f[...].astype(BF)

        lane = lax.broadcasted_iota(jnp.int32, (64, 128), 1)
        lo = lane < 64
        r128 = lax.broadcasted_iota(jnp.int32, (128, 128), 0)
        c128 = lax.broadcasted_iota(jnp.int32, (128, 128), 1)
        dmask = (r128 < 64) == (c128 < 64)
        NEG = jnp.float32(-jnp.inf)

        def softmax_seg(s):
            m_lo = jnp.max(jnp.where(lo, s, NEG), axis=-1, keepdims=True)
            m_hi = jnp.max(jnp.where(lo, NEG, s), axis=-1, keepdims=True)
            p = jnp.exp(s - jnp.where(lo, m_lo, m_hi))
            l_lo = jnp.sum(jnp.where(lo, p, 0.0), axis=-1, keepdims=True)
            l_hi = jnp.sum(jnp.where(lo, 0.0, p), axis=-1, keepdims=True)
            return (p * jnp.where(lo, 1.0 / l_lo, 1.0 / l_hi)).astype(BF)

        def attn(s, q):
            qp = jnp.dot(x_b[...], wq_all[s, q], preferred_element_type=F32) * 0.125
            kv_ld[(s, q)][0].wait()
            kv_ld[(s, q)][1].wait()
            for b in range(2):
                for g in range(2):
                    r0 = b * 256 + g * 128
                    qa = qp[r0:r0 + 64]
                    qb = qp[r0 + 64:r0 + 128]
                    l1 = jnp.where(lo, qa, qb).astype(BF)
                    l2 = jnp.where(lo, qb, qa).astype(BF)
                    kk = kt_f[s, q, b, :, g * 128:(g + 1) * 128]
                    vv = vt_f[s, q, b, :, g * 128:(g + 1) * 128]
                    m1 = jnp.where(dmask, kk, 0.0).astype(BF)
                    m2 = jnp.where(dmask, 0.0, kk).astype(BF)
                    v1 = jnp.where(dmask, vv, 0.0).astype(BF)
                    v2 = jnp.where(dmask, 0.0, vv).astype(BF)
                    p1 = softmax_seg(jnp.dot(l1, m1, preferred_element_type=F32))
                    p2 = softmax_seg(jnp.dot(l2, m2, preferred_element_type=F32))
                    nt = (((1,), (1,)), ((), ()))
                    c1 = lax.dot_general(p1, v1, nt, preferred_element_type=F32)
                    c2 = lax.dot_general(p2, v2, nt, preferred_element_type=F32)
                    ctx[s, q, r0:r0 + 64, :] = jnp.where(lo, c1, c2).astype(BF)
                    ctx[s, q, r0 + 64:r0 + 128, :] = jnp.where(lo, c2, c1).astype(BF)

        def wo_tile(s, q, n):
            if n < 3:
                return wo_all[s, q, n * 128:(n + 1) * 128, :]
            r = 384 + 64 * q
            return jnp.concatenate([wo_all[s, 0, r:r + 64, :], wo_all[s, 1, r:r + 64, :]], axis=0)

        def oproj(terms, n, first=False, last=False, split=1):
            rows = T // split
            ws = [wo_tile(s, q, n) for (s, q) in terms]
            for i in range(split):
                rs = slice(i * rows, (i + 1) * rows)
                r = None if first else acc[n, rs, :]
                for (s, q), w in zip(terms, ws):
                    t = jnp.dot(ctx[s, q, rs, :], w, preferred_element_type=F32)
                    r = t if r is None else r + t
                if last:
                    out_ref[rs, n * 128:(n + 1) * 128] = r.astype(out_ref.dtype)
                else:
                    acc[n, rs, :] = r

        with scope("attn00"):
            attn(0, 0)
        with scope("wo_cast"):
            wo_ld.wait()
            for q in range(2):
                for n in range(3):
                    wo_all[0, q, n * 128:(n + 1) * 128, :] = wo_f[q * 128:(q + 1) * 128, n * 128:(n + 1) * 128].astype(BF)
                for d in range(2):
                    wo_all[0, d, 384 + 64 * q:448 + 64 * q, :] = wo_f[q * 128 + d * 64:q * 128 + d * 64 + 64, 384:512].astype(BF)
        b1a = [rcopy(wo_all.at[0, d, pl.ds(0, 256)], wo_all.at[1 + d, d, pl.ds(0, 256)], d) for d in range(2)]
        with scope("attn01"):
            attn(0, 1)

        with scope("wait_a1"):
            for cp in a1[0] + a1[1]:
                cp.wait_recv()
        fq = [rcopy(wq_all.at[1 + d, d], wq_all.at[3, d], d) for d in range(2)]
        b1b = [rcopy(wo_all.at[0, d, pl.ds(256, 256)], wo_all.at[1 + d, d, pl.ds(256, 256)], d) for d in range(2)]
        b2 = [rcopy(wo_all.at[0, 1 - d], wo_all.at[1 + d, 1 - d], d) for d in range(2)]

        with scope("attn10"):
            attn(1, 0)
        with scope("attn21"):
            attn(2, 1)
        with scope("wait_a2"):
            for d in range(2):
                a2[d].wait_recv()
        with scope("attn11"):
            attn(1, 1)
        with scope("attn20"):
            attn(2, 0)
        with scope("wait_b1a"):
            for d in range(2):
                b1a[d].wait_recv()
        FO = ((0, 128), (128, 128), (256, 128), (384, 64), (448, 64))
        fo = []
        for (o, n) in FO[:2]:
            fo.append([rcopy(wo_all.at[1 + d, d, pl.ds(o, n)], wo_all.at[3, d, pl.ds(o, n)], d) for d in range(2)])
        with scope("oproj0"):
            for n in range(2):
                oproj(((0, 0), (0, 1), (1, 0), (2, 1)), n, first=True)
            for n in range(2, 4):
                oproj(((0, 0), (0, 1)), n, first=True)
        with scope("wait_fq"):
            for d in range(2):
                fq[d].wait_recv()
        with scope("attn30"):
            attn(3, 0)
        with scope("attn31"):
            attn(3, 1)
        with scope("wait_b1b"):
            for d in range(2):
                b1b[d].wait_recv()
        for (o, n) in FO[2:]:
            fo.append([rcopy(wo_all.at[1 + d, d, pl.ds(o, n)], wo_all.at[3, d, pl.ds(o, n)], d) for d in range(2)])
        with scope("oproj_b1b"):
            oproj(((1, 0), (2, 1)), 2)
        with scope("wait_b2"):
            for d in range(2):
                b2[d].wait_recv()
        with scope("oproj_b2"):
            for n in range(3):
                oproj(((1, 1), (2, 0)), n)
            oproj(((1, 0), (1, 1), (2, 0), (2, 1)), 3)
        for n in range(3):
            with scope(f"wait_fo{n}"):
                for d in range(2):
                    fo[n][d].wait_recv()
            with scope(f"oproj_f{n}"):
                oproj(((3, 0), (3, 1)), n, last=True, split=2)
        with scope("wait_fo3"):
            for d in range(2):
                fo[3][d].wait_recv()
        with scope("oproj_f3"):
            oproj(((3, 0),), 3, split=4)
        with scope("sends"):
            for cp in sends:
                cp.wait_send()
        with scope("wait_fo4"):
            for d in range(2):
                fo[4][d].wait_recv()
        with scope("oproj_f4"):
            oproj(((3, 1),), 3, last=True, split=4)

    anyspec = pl.BlockSpec(memory_space=pl.ANY)
    out = pl.pallas_call(
        body,
        out_shape=jax.ShapeDtypeStruct((T, D), OUT_DTYPE),
        in_specs=[anyspec] * 5,
        out_specs=pl.BlockSpec(memory_space=pltpu.VMEM),
        scratch_shapes=[
            pltpu.VMEM((T, D), F32),
            pltpu.VMEM((512, 256), F32),
            pltpu.VMEM((256, 512), F32),
            pltpu.VMEM((4, 2, 2, 128, 256), F32),
            pltpu.VMEM((4, 2, 2, 128, 256), F32),
            pltpu.VMEM((T, D), BF),
            pltpu.VMEM((4, 2, 512, 128), BF),
            pltpu.VMEM((4, 2, 512, 128), BF),
            pltpu.VMEM((4, 2, T, 128), BF),
            pltpu.VMEM((4, T, 128), F32),
            pltpu.SemaphoreType.DMA((24,)),
            pltpu.SemaphoreType.DMA((32,)),
            pltpu.SemaphoreType.DMA((32,)),
            pltpu.SemaphoreType.REGULAR,
        ],
        compiler_params=pltpu.CompilerParams(
            collective_id=0, vmem_limit_bytes=64 * 1024 * 1024,
            disable_semaphore_checks=not CHECKS, disable_bounds_checks=not CHECKS),
    )(x2, Wq, KT, VT, Wo)
    return out.reshape(2, 256, D)
```

```python
import jax
import jax.numpy as jnp
from jax import lax
from jax.experimental import pallas as pl
from jax.experimental.pallas import tpu as pltpu

N_DEV = 4
T = 512
D = 512
BF = jnp.bfloat16
F32 = jnp.float32

WQ_CHUNKS = ((0, 48), (48, 80), (128, 128), (256, 256))
HEAD_ROWS = 32
FWD_WO = ((0, 128), (128, 128), (256, 128), (384, 64), (448, 64))

N_LOCAL = len(WQ_CHUNKS) + 2 + 16
N_REMOTE = 2 * (1 + len(WQ_CHUNKS) + 1 + 1 + 3 + len(FWD_WO))


def _compiler_params():
    base = dict(collective_id=0, vmem_limit_bytes=64 * 1024 * 1024)
    try:
        return pltpu.CompilerParams(disable_semaphore_checks=True, **base)
    except TypeError:
        return pltpu.CompilerParams(**base)


def _body(x_hbm, wq_hbm, kt_hbm, vt_hbm, wo_hbm, out_ref,
          x_f, wq_f, wo_f, kt_f, vt_f,
          x_b, wq_all, wo_all, ctx, acc, head_buf,
          lsem, ssem, rsem, rdy):
    mesh_id = pl.DeviceIdType.MESH
    me = lax.axis_index("i")
    right = lax.rem(me + 1, N_DEV)
    left = lax.rem(me + 3, N_DEV)
    diag = lax.rem(me + 2, N_DEV)
    nbr = (right, left)
    slot_group = (me, left, right, diag)

    counts = {"local": 0, "remote": 0}
    sends = []

    def load(src, dst):
        cp = pltpu.make_async_copy(src, dst, lsem.at[counts["local"]])
        counts["local"] += 1
        cp.start()
        return cp

    def remote_descs(srcs, dst, d):
        i = counts["remote"]
        counts["remote"] += 1
        cps = [pltpu.make_async_remote_copy(s, dst, ssem.at[i], rsem.at[i],
                                            device_id=(nbr[d],), device_id_type=mesh_id)
               for s in srcs]
        sends.append(cps[0])
        return cps

    def remote(src, dst, d):
        return remote_descs([src], dst, d)[0]

    def send(src, dst, d):
        cp = remote(src, dst, d)
        cp.start()
        return cp

    def load_wq(chunks):
        return [load(wq_hbm.at[pl.ds(o, n)], wq_f.at[pl.ds(o, n)]) for o, n in chunks]

    wq_ld = load_wq(WQ_CHUNKS[:2])

    head_hbm, head_vmem = [], []
    for d in range(2):
        idx = (pl.ds(0, HEAD_ROWS), pl.ds((1 - d) * 128, 128))
        a, b = remote_descs([wq_hbm.at[idx], wq_f.at[idx]], head_buf.at[d], d)
        head_hbm.append(a)
        head_vmem.append(b)

    bar = pltpu.get_barrier_semaphore()

    @pl.when(me != 2)
    def _():
        for n in nbr:
            pl.semaphore_signal(bar, inc=1, device_id=(n,), device_id_type=mesh_id)

    for pos, d in ((1, 1), (3, 0)):
        @pl.when(me == pos)
        def _():
            pl.semaphore_wait(bar, 1)
            head_hbm[d].start()

    @pl.when(me == 2)
    def _():
        pl.semaphore_wait(bar, 2)
        for n in nbr:
            pl.semaphore_signal(rdy, inc=1, device_id=(n,), device_id_type=mesh_id)
        for d in range(2):
            head_hbm[d].start()

    wq_ld += load_wq(WQ_CHUNKS[2:])

    rest = pl.ds(HEAD_ROWS, D - HEAD_ROWS)
    wq_first = [[remote(wq_all.at[0, d, pl.ds(o, n)], wq_all.at[1 + d, d, pl.ds(o, n)], d)
                 for o, n in WQ_CHUNKS] for d in range(2)]
    wq_second = [remote(wq_all.at[0, 1 - d, rest], wq_all.at[1 + d, 1 - d, rest], d)
                 for d in range(2)]
    link_open = (me >= 2, jnp.logical_or(me == 1, me == 2))

    def load_kv(s, q):
        src = (pl.ds(2 * me, 2), slot_group[s] * 2 + q)
        return load(kt_hbm.at[src], kt_f.at[s, q]), load(vt_hbm.at[src], vt_f.at[s, q])

    kv_ld = {}
    for ci, (o, n) in enumerate(WQ_CHUNKS):
        wq_ld[ci].wait()
        for q in range(2):
            wq_all[0, q, o:o + n, :] = wq_f[o:o + n, q * 128:(q + 1) * 128].astype(BF)
        for d in range(2):
            @pl.when(link_open[d])
            def _():
                wq_first[d][ci].start()
                if ci == len(WQ_CHUNKS) - 1:
                    wq_second[d].start()
        if ci == 0:
            x_ld = load(x_hbm, x_f)
            kv_ld[(0, 0)] = load_kv(0, 0)
            wo_ld = load(wo_hbm, wo_f)
            for sq in ((0, 1), (1, 0), (2, 1), (1, 1), (2, 0), (3, 0), (3, 1)):
                kv_ld[sq] = load_kv(*sq)

    def late_start(d):
        head_vmem[d].start()
        for cp in wq_first[d]:
            cp.start()
        wq_second[d].start()

    @pl.when(me == 0)
    def _():
        pl.semaphore_wait(bar, 2)
        late_start(0)
        late_start(1)

    for pos, d in ((1, 0), (3, 1)):
        @pl.when(me == pos)
        def _():
            pl.semaphore_wait(rdy, 1)
            late_start(d)

    x_ld.wait()
    x_b[...] = x_f[...].astype(BF)

    lo = lax.broadcasted_iota(jnp.int32, (64, 128), 1) < 64
    on_diag = ((lax.broadcasted_iota(jnp.int32, (128, 128), 0) < 64)
               == (lax.broadcasted_iota(jnp.int32, (128, 128), 1) < 64))
    neg = jnp.float32(-jnp.inf)

    def softmax_halves(s):
        m_lo = jnp.max(jnp.where(lo, s, neg), axis=-1, keepdims=True)
        m_hi = jnp.max(jnp.where(lo, neg, s), axis=-1, keepdims=True)
        p = jnp.exp(s - jnp.where(lo, m_lo, m_hi))
        l_lo = jnp.sum(jnp.where(lo, p, 0.0), axis=-1, keepdims=True)
        l_hi = jnp.sum(jnp.where(lo, 0.0, p), axis=-1, keepdims=True)
        return (p * jnp.where(lo, 1.0 / l_lo, 1.0 / l_hi)).astype(BF)

    def attend(s, q, kv_wait_first=True):
        def wait_kv():
            for cp in kv_ld[(s, q)]:
                cp.wait()

        if kv_wait_first:
            wait_kv()
        qp = jnp.dot(x_b[...], wq_all[s, q], preferred_element_type=F32) * 0.125
        if not kv_wait_first:
            wait_kv()
        nt = (((1,), (1,)), ((), ()))
        for b in range(2):
            for g in range(2):
                r0 = b * 256 + g * 128
                qa = qp[r0:r0 + 64]
                qb = qp[r0 + 64:r0 + 128]
                kk = kt_f[s, q, b, :, g * 128:(g + 1) * 128]
                vv = vt_f[s, q, b, :, g * 128:(g + 1) * 128]
                s1 = jnp.dot(jnp.where(lo, qa, qb).astype(BF),
                             jnp.where(on_diag, kk, 0.0).astype(BF),
                             preferred_element_type=F32)
                s2 = jnp.dot(jnp.where(lo, qb, qa).astype(BF),
                             jnp.where(on_diag, 0.0, kk).astype(BF),
                             preferred_element_type=F32)
                c1 = lax.dot_general(softmax_halves(s1),
                                     jnp.where(on_diag, vv, 0.0).astype(BF),
                                     nt, preferred_element_type=F32)
                c2 = lax.dot_general(softmax_halves(s2),
                                     jnp.where(on_diag, 0.0, vv).astype(BF),
                                     nt, preferred_element_type=F32)
                ctx[s, q, r0:r0 + 64, :] = jnp.where(lo, c1, c2).astype(BF)
                ctx[s, q, r0 + 64:r0 + 128, :] = jnp.where(lo, c2, c1).astype(BF)

    def wo_tile(s, q, n):
        if n < 3:
            return wo_all[s, q, n * 128:(n + 1) * 128, :]
        r = 384 + 64 * q
        return jnp.concatenate([wo_all[s, 0, r:r + 64, :], wo_all[s, 1, r:r + 64, :]], axis=0)

    def project(terms, n, first=False, last=False, split=1):
        rows = T // split
        tiles = [wo_tile(s, q, n) for s, q in terms]
        for i in range(split):
            rs = slice(i * rows, (i + 1) * rows)
            r = None if first else acc[n, rs, :]
            for (s, q), w in zip(terms, tiles):
                t = jnp.dot(ctx[s, q, rs, :], w, preferred_element_type=F32)
                r = t if r is None else r + t
            if last:
                out_ref[rs, n * 128:(n + 1) * 128] = r
            else:
                acc[n, rs, :] = r

    def wait_recv(cps):
        for cp in cps:
            cp.wait_recv()

    def send_wo(src_slot, dst_slot, stream, rows):
        return [send(wo_all.at[src_slot(d), stream(d), rows],
                     wo_all.at[dst_slot(d), stream(d), rows], d) for d in range(2)]

    def send_own_wo(stream, rows):
        return send_wo(lambda d: 0, lambda d: 1 + d, stream, rows)

    def forward_wo(o, n):
        return send_wo(lambda d: 1 + d, lambda d: 3, lambda d: d, pl.ds(o, n))

    attend(0, 0, kv_wait_first=False)
    wo_ld.wait()
    for q in range(2):
        for n in range(3):
            wo_all[0, q, n * 128:(n + 1) * 128, :] = (
                wo_f[q * 128:(q + 1) * 128, n * 128:(n + 1) * 128].astype(BF))
        for d in range(2):
            r = q * 128 + d * 64
            wo_all[0, d, 384 + 64 * q:448 + 64 * q, :] = wo_f[r:r + 64, 384:512].astype(BF)
    wo_first_a = send_own_wo(lambda d: d, pl.ds(0, 256))
    attend(0, 1, kv_wait_first=False)

    wait_recv(wq_first[0] + wq_first[1])
    wq_fwd = [send(wq_all.at[1 + d, d], wq_all.at[3, d], d) for d in range(2)]
    wo_first_b = send_own_wo(lambda d: d, pl.ds(256, 256))
    n_done_early = len(sends)
    wo_second = send_own_wo(lambda d: 1 - d, pl.ds(0, 512))
    attend(1, 0)
    attend(2, 1)

    for d in range(2):
        head_hbm[d].wait_recv()
        wq_all[1 + d, 1 - d, 0:HEAD_ROWS, :] = head_buf[d].astype(BF)
    wait_recv(wq_second)
    attend(1, 1)
    attend(2, 0)

    wait_recv(wo_first_a)
    wo_fwd = [forward_wo(o, n) for o, n in FWD_WO[:2]]
    for n in range(2):
        project(((0, 0), (0, 1), (1, 0), (2, 1)), n, first=True)
    for n in range(2, 4):
        project(((0, 0), (0, 1)), n, first=True)

    wait_recv(wq_fwd)
    attend(3, 0)
    attend(3, 1)

    wait_recv(wo_first_b)
    wo_fwd += [forward_wo(o, n) for o, n in FWD_WO[2:]]
    project(((1, 0), (2, 1)), 2, split=2)
    for cp in sends[:n_done_early]:
        cp.wait_send()

    wait_recv(wo_second)
    for n in range(3):
        project(((1, 1), (2, 0)), n)
    project(((1, 0), (1, 1), (2, 0), (2, 1)), 3)

    for n in range(3):
        wait_recv(wo_fwd[n])
        project(((3, 0), (3, 1)), n, last=True, split=2)
    wait_recv(wo_fwd[3])
    project(((3, 0),), 3, split=4)
    for cp in sends[n_done_early:]:
        cp.wait_send()
    wait_recv(wo_fwd[4])
    project(((3, 1),), 3, last=True, split=4)

    assert counts["local"] == N_LOCAL and counts["remote"] == N_REMOTE


def pallas_dist_sparse_attn_strided_htp_bs_b2_sq256_skv256_hq4_dh64_kernel(
    x: jax.Array,
    Wq: jax.Array,
    K_ext: jax.Array,
    V_ext: jax.Array,
    Wo: jax.Array,
):
    kt = jnp.transpose(K_ext, (0, 2, 3, 1)).reshape(8, 8, 128, 256)
    vt = jnp.transpose(V_ext, (0, 2, 3, 1)).reshape(8, 8, 128, 256)

    out = pl.pallas_call(
        _body,
        out_shape=jax.ShapeDtypeStruct((T, D), F32),
        in_specs=[pl.BlockSpec(memory_space=pl.ANY)] * 5,
        out_specs=pl.BlockSpec(memory_space=pltpu.VMEM),
        scratch_shapes=[
            pltpu.VMEM((T, D), F32),
            pltpu.VMEM((512, 256), F32),
            pltpu.VMEM((256, 512), F32),
            pltpu.VMEM((4, 2, 2, 128, 256), F32),
            pltpu.VMEM((4, 2, 2, 128, 256), F32),
            pltpu.VMEM((T, D), BF),
            pltpu.VMEM((4, 2, 512, 128), BF),
            pltpu.VMEM((4, 2, 512, 128), BF),
            pltpu.VMEM((4, 2, T, 128), BF),
            pltpu.VMEM((4, T, 128), F32),
            pltpu.VMEM((2, HEAD_ROWS, 128), F32),
            pltpu.SemaphoreType.DMA((N_LOCAL,)),
            pltpu.SemaphoreType.DMA((N_REMOTE,)),
            pltpu.SemaphoreType.DMA((N_REMOTE,)),
            pltpu.SemaphoreType.REGULAR,
        ],
        compiler_params=_compiler_params(),
    )(x.reshape(T, D), Wq, kt, vt, Wo)
    return out.reshape(2, 256, D)
```

```python
import jax
import jax.numpy as jnp
from jax import lax
from jax.experimental import pallas as pl
from jax.experimental.pallas import tpu as pltpu

N_DEV = 4
T = 512
D = 512
BF = jnp.bfloat16
F32 = jnp.float32

WQ_CHUNKS = ((0, 48), (48, 80), (128, 128), (256, 256))
HEAD_ROWS = 32
FWD_WO = ((0, 128), (128, 128), (256, 128), (384, 64), (448, 64))

N_LOCAL = len(WQ_CHUNKS) + 2 + 16
N_REMOTE = 2 * (1 + len(WQ_CHUNKS) + 1 + 1 + 3 + len(FWD_WO))


def _body(x_hbm, wq_hbm, kt_hbm, vt_hbm, wo_hbm, out_ref,
          x_f, wq_f, wo_f, kt_f, vt_f,
          x_b, wq_all, wo_all, ctx, acc, head_buf,
          lsem, ssem, rsem, rdy):
    mesh_id = pl.DeviceIdType.MESH
    me = lax.axis_index("i")
    right = lax.rem(me + 1, N_DEV)
    left = lax.rem(me + 3, N_DEV)
    diag = lax.rem(me + 2, N_DEV)
    nbr = (right, left)
    slot_group = (me, left, right, diag)

    counts = {"local": 0, "remote": 0}
    sends = []

    def load(src, dst):
        cp = pltpu.make_async_copy(src, dst, lsem.at[counts["local"]])
        counts["local"] += 1
        cp.start()
        return cp

    def remote_descs(srcs, dst, d):
        i = counts["remote"]
        counts["remote"] += 1
        cps = [pltpu.make_async_remote_copy(s, dst, ssem.at[i], rsem.at[i],
                                            device_id=(nbr[d],), device_id_type=mesh_id)
               for s in srcs]
        sends.append(cps[0])
        return cps

    def remote(src, dst, d):
        return remote_descs([src], dst, d)[0]

    def send(src, dst, d):
        cp = remote(src, dst, d)
        cp.start()
        return cp

    def load_wq(chunks):
        return [load(wq_hbm.at[pl.ds(o, n)], wq_f.at[pl.ds(o, n)]) for o, n in chunks]

    wq_ld = load_wq(WQ_CHUNKS[:2])

    head_hbm, head_vmem = [], []
    for d in range(2):
        idx = (pl.ds(0, HEAD_ROWS), pl.ds((1 - d) * 128, 128))
        a, b = remote_descs([wq_hbm.at[idx], wq_f.at[idx]], head_buf.at[d], d)
        head_hbm.append(a)
        head_vmem.append(b)

    bar = pltpu.get_barrier_semaphore()

    @pl.when(me != 2)
    def _():
        for n in nbr:
            pl.semaphore_signal(bar, inc=1, device_id=(n,), device_id_type=mesh_id)

    for pos, d in ((1, 1), (3, 0)):
        @pl.when(me == pos)
        def _():
            pl.semaphore_wait(bar, 1)
            head_hbm[d].start()

    @pl.when(me == 2)
    def _():
        pl.semaphore_wait(bar, 2)
        for n in nbr:
            pl.semaphore_signal(rdy, inc=1, device_id=(n,), device_id_type=mesh_id)
        for d in range(2):
            head_hbm[d].start()

    wq_ld += load_wq(WQ_CHUNKS[2:])

    rest = pl.ds(HEAD_ROWS, D - HEAD_ROWS)
    wq_first = [[remote(wq_all.at[0, d, pl.ds(o, n)], wq_all.at[1 + d, d, pl.ds(o, n)], d)
                 for o, n in WQ_CHUNKS] for d in range(2)]
    wq_second = [remote(wq_all.at[0, 1 - d, rest], wq_all.at[1 + d, 1 - d, rest], d)
                 for d in range(2)]
    link_open = (me >= 2, jnp.logical_or(me == 1, me == 2))

    def load_kv(s, q):
        src = (pl.ds(2 * me, 2), slot_group[s] * 2 + q)
        return load(kt_hbm.at[src], kt_f.at[s, q]), load(vt_hbm.at[src], vt_f.at[s, q])

    kv_ld = {}
    for ci, (o, n) in enumerate(WQ_CHUNKS):
        wq_ld[ci].wait()
        for q in range(2):
            wq_all[0, q, o:o + n, :] = wq_f[o:o + n, q * 128:(q + 1) * 128].astype(BF)
        for d in range(2):
            @pl.when(link_open[d])
            def _():
                wq_first[d][ci].start()
                if ci == len(WQ_CHUNKS) - 1:
                    wq_second[d].start()
        if ci == 0:
            x_ld = load(x_hbm, x_f)
            kv_ld[(0, 0)] = load_kv(0, 0)
            wo_ld = load(wo_hbm, wo_f)
            for sq in ((0, 1), (1, 0), (2, 1), (1, 1), (2, 0), (3, 0), (3, 1)):
                kv_ld[sq] = load_kv(*sq)

    def late_start(d):
        head_vmem[d].start()
        for cp in wq_first[d]:
            cp.start()
        wq_second[d].start()

    @pl.when(me == 0)
    def _():
        pl.semaphore_wait(bar, 2)
        late_start(0)
        late_start(1)

    for pos, d in ((1, 0), (3, 1)):
        @pl.when(me == pos)
        def _():
            pl.semaphore_wait(rdy, 1)
            late_start(d)

    x_ld.wait()
    x_b[...] = x_f[...].astype(BF)

    lo = lax.broadcasted_iota(jnp.int32, (64, 128), 1) < 64
    on_diag = ((lax.broadcasted_iota(jnp.int32, (128, 128), 0) < 64)
               == (lax.broadcasted_iota(jnp.int32, (128, 128), 1) < 64))
    neg = jnp.float32(-jnp.inf)

    def softmax_halves(s):
        m_lo = jnp.max(jnp.where(lo, s, neg), axis=-1, keepdims=True)
        m_hi = jnp.max(jnp.where(lo, neg, s), axis=-1, keepdims=True)
        p = jnp.exp(s - jnp.where(lo, m_lo, m_hi))
        l_lo = jnp.sum(jnp.where(lo, p, 0.0), axis=-1, keepdims=True)
        l_hi = jnp.sum(jnp.where(lo, 0.0, p), axis=-1, keepdims=True)
        return (p * jnp.where(lo, 1.0 / l_lo, 1.0 / l_hi)).astype(BF)

    def attend(s, q, kv_wait_first=True):
        def wait_kv():
            for cp in kv_ld[(s, q)]:
                cp.wait()

        if kv_wait_first:
            wait_kv()
        qp = jnp.dot(x_b[...], wq_all[s, q], preferred_element_type=F32) * 0.125
        if not kv_wait_first:
            wait_kv()
        nt = (((1,), (1,)), ((), ()))
        for b in range(2):
            for g in range(2):
                r0 = b * 256 + g * 128
                qa = qp[r0:r0 + 64]
                qb = qp[r0 + 64:r0 + 128]
                kk = kt_f[s, q, b, :, g * 128:(g + 1) * 128]
                vv = vt_f[s, q, b, :, g * 128:(g + 1) * 128]
                s1 = jnp.dot(jnp.where(lo, qa, qb).astype(BF),
                             jnp.where(on_diag, kk, 0.0).astype(BF),
                             preferred_element_type=F32)
                s2 = jnp.dot(jnp.where(lo, qb, qa).astype(BF),
                             jnp.where(on_diag, 0.0, kk).astype(BF),
                             preferred_element_type=F32)
                c1 = lax.dot_general(softmax_halves(s1),
                                     jnp.where(on_diag, vv, 0.0).astype(BF),
                                     nt, preferred_element_type=F32)
                c2 = lax.dot_general(softmax_halves(s2),
                                     jnp.where(on_diag, 0.0, vv).astype(BF),
                                     nt, preferred_element_type=F32)
                ctx[s, q, r0:r0 + 64, :] = jnp.where(lo, c1, c2).astype(BF)
                ctx[s, q, r0 + 64:r0 + 128, :] = jnp.where(lo, c2, c1).astype(BF)

    def wo_tile(s, q, n):
        if n < 3:
            return wo_all[s, q, n * 128:(n + 1) * 128, :]
        r = 384 + 64 * q
        return jnp.concatenate([wo_all[s, 0, r:r + 64, :], wo_all[s, 1, r:r + 64, :]], axis=0)

    def project(terms, n, first=False, last=False, split=1):
        rows = T // split
        tiles = [wo_tile(s, q, n) for s, q in terms]
        for i in range(split):
            rs = slice(i * rows, (i + 1) * rows)
            r = None if first else acc[n, rs, :]
            for (s, q), w in zip(terms, tiles):
                t = jnp.dot(ctx[s, q, rs, :], w, preferred_element_type=F32)
                r = t if r is None else r + t
            if last:
                out_ref[rs, n * 128:(n + 1) * 128] = r
            else:
                acc[n, rs, :] = r

    def wait_recv(cps):
        for cp in cps:
            cp.wait_recv()

    def send_wo(src_slot, dst_slot, stream, rows):
        return [send(wo_all.at[src_slot(d), stream(d), rows],
                     wo_all.at[dst_slot(d), stream(d), rows], d) for d in range(2)]

    def send_own_wo(stream, rows):
        return send_wo(lambda d: 0, lambda d: 1 + d, stream, rows)

    def forward_wo(o, n):
        return send_wo(lambda d: 1 + d, lambda d: 3, lambda d: d, pl.ds(o, n))

    attend(0, 0, kv_wait_first=False)
    wo_ld.wait()
    for q in range(2):
        for n in range(3):
            wo_all[0, q, n * 128:(n + 1) * 128, :] = (
                wo_f[q * 128:(q + 1) * 128, n * 128:(n + 1) * 128].astype(BF))
        for d in range(2):
            r = q * 128 + d * 64
            wo_all[0, d, 384 + 64 * q:448 + 64 * q, :] = wo_f[r:r + 64, 384:512].astype(BF)
    wo_first_a = send_own_wo(lambda d: d, pl.ds(0, 256))
    attend(0, 1, kv_wait_first=False)

    wait_recv(wq_first[0] + wq_first[1])
    wq_fwd = [send(wq_all.at[1 + d, d], wq_all.at[3, d], d) for d in range(2)]
    wo_first_b = send_own_wo(lambda d: d, pl.ds(256, 256))
    n_done_early = len(sends)
    wo_second = send_own_wo(lambda d: 1 - d, pl.ds(0, 512))
    attend(1, 0)
    attend(2, 1)

    wait_recv(head_hbm + wq_second)
    for d in range(2):
        wq_all[1 + d, 1 - d, 0:HEAD_ROWS, :] = head_buf[d].astype(BF)
    attend(1, 1)
    attend(2, 0)

    wait_recv(wo_first_a)
    wo_fwd = [forward_wo(o, n) for o, n in FWD_WO[:2]]
    for n in range(2):
        project(((0, 0), (0, 1), (1, 0), (2, 1)), n, first=True)
    for n in range(2, 4):
        project(((0, 0), (0, 1)), n, first=True)

    wait_recv(wq_fwd)
    attend(3, 0)
    attend(3, 1)

    wait_recv(wo_first_b)
    wo_fwd += [forward_wo(o, n) for o, n in FWD_WO[2:]]
    project(((1, 0), (2, 1)), 2, split=2)
    for cp in sends[:n_done_early]:
        cp.wait_send()

    wait_recv(wo_second)
    for n in range(3):
        project(((1, 1), (2, 0)), n)
    project(((1, 0), (1, 1), (2, 0), (2, 1)), 3)

    for n in range(3):
        wait_recv(wo_fwd[n])
        project(((3, 0), (3, 1)), n, last=True, split=2)
    wait_recv(wo_fwd[3])
    project(((3, 0),), 3, split=4)
    for cp in sends[n_done_early:]:
        cp.wait_send()
    wait_recv(wo_fwd[4])
    project(((3, 1),), 3, last=True, split=4)

    assert counts["local"] == N_LOCAL and counts["remote"] == N_REMOTE


def _kernel(*refs):
    pl.run_scoped(
        lambda *sems: _body(*refs, *sems),
        pltpu.SemaphoreType.DMA((N_LOCAL,)),
        pltpu.SemaphoreType.DMA((N_REMOTE,)),
        pltpu.SemaphoreType.DMA((N_REMOTE,)),
        pltpu.SemaphoreType.REGULAR,
    )


def pallas_dist_sparse_attn_strided_htp_bs_b2_sq256_skv256_hq4_dh64_kernel(
    x: jax.Array,
    Wq: jax.Array,
    K_ext: jax.Array,
    V_ext: jax.Array,
    Wo: jax.Array,
):
    kt = jnp.transpose(K_ext, (0, 2, 3, 1)).reshape(8, 8, 128, 256)
    vt = jnp.transpose(V_ext, (0, 2, 3, 1)).reshape(8, 8, 128, 256)

    out = pl.pallas_call(
        _kernel,
        out_shape=jax.ShapeDtypeStruct((T, D), F32),
        in_specs=[pl.BlockSpec(memory_space=pl.ANY)] * 5,
        out_specs=pl.BlockSpec(memory_space=pltpu.VMEM),
        scratch_shapes=[
            pltpu.VMEM((T, D), F32),
            pltpu.VMEM((512, 256), F32),
            pltpu.VMEM((256, 512), F32),
            pltpu.VMEM((4, 2, 2, 128, 256), F32),
            pltpu.VMEM((4, 2, 2, 128, 256), F32),
            pltpu.VMEM((T, D), BF),
            pltpu.VMEM((4, 2, 512, 128), BF),
            pltpu.VMEM((4, 2, 512, 128), BF),
            pltpu.VMEM((4, 2, T, 128), BF),
            pltpu.VMEM((4, T, 128), F32),
            pltpu.VMEM((2, HEAD_ROWS, 128), F32),
        ],
        compiler_params=pltpu.CompilerParams(
            collective_id=0, vmem_limit_bytes=64 * 1024 * 1024),
    )(x.reshape(T, D), Wq, kt, vt, Wo)
    return out.reshape(2, 256, D)
```

```python
import jax
import jax.numpy as jnp
from jax import lax
from jax.experimental import pallas as pl
from jax.experimental.pallas import tpu as pltpu

N_DEV = 4
T = 512
D = 512
BF = jnp.bfloat16
F32 = jnp.float32

WQ_CHUNKS = ((0, 16), (16, 48), (64, 64), (128, 128), (256, 256))
HEAD_ROWS = 32
FWD_WO = ((0, 128), (128, 128), (256, 128), (384, 64), (448, 64))

N_LOCAL = len(WQ_CHUNKS) + 2 + 16
N_REMOTE = 2 * (1 + len(WQ_CHUNKS) + 1 + 1 + 3 + len(FWD_WO))


def _body(x_hbm, wq_hbm, kt_hbm, vt_hbm, wo_hbm, out_ref,
          x_f, wq_f, wo_f, kt_f, vt_f,
          x_b, wq_all, wo_all, ctx, acc, head_buf,
          lsem, ssem, rsem, rdy):
    mesh_id = pl.DeviceIdType.MESH
    me = lax.axis_index("i")
    right = lax.rem(me + 1, N_DEV)
    left = lax.rem(me + 3, N_DEV)
    diag = lax.rem(me + 2, N_DEV)
    nbr = (right, left)
    slot_group = (me, left, right, diag)

    counts = {"local": 0, "remote": 0}
    sends = []

    def load(src, dst):
        cp = pltpu.make_async_copy(src, dst, lsem.at[counts["local"]])
        counts["local"] += 1
        cp.start()
        return cp

    def remote(src, dst, d):
        i = counts["remote"]
        counts["remote"] += 1
        cp = pltpu.make_async_remote_copy(src, dst, ssem.at[i], rsem.at[i],
                                          device_id=(nbr[d],), device_id_type=mesh_id)
        sends.append(cp)
        return cp

    def send(src, dst, d):
        cp = remote(src, dst, d)
        cp.start()
        return cp

    def load_wq(chunks):
        return [load(wq_hbm.at[pl.ds(o, n)], wq_f.at[pl.ds(o, n)]) for o, n in chunks]

    wq_ld = load_wq(WQ_CHUNKS[:2])

    head = [remote(wq_hbm.at[pl.ds(0, HEAD_ROWS), pl.ds((1 - d) * 128, 128)], head_buf.at[d], d)
            for d in range(2)]

    bar = pltpu.get_barrier_semaphore()

    @pl.when(me != 2)
    def _():
        for n in nbr:
            pl.semaphore_signal(bar, inc=1, device_id=(n,), device_id_type=mesh_id)

    for pos, d in ((1, 1), (3, 0)):
        @pl.when(me == pos)
        def _():
            pl.semaphore_wait(bar, 1)
            head[d].start()

    @pl.when(me == 2)
    def _():
        pl.semaphore_wait(bar, 2)
        for n in nbr:
            pl.semaphore_signal(rdy, inc=1, device_id=(n,), device_id_type=mesh_id)
        for d in range(2):
            head[d].start()

    wq_ld += load_wq(WQ_CHUNKS[2:])

    rest = pl.ds(HEAD_ROWS, D - HEAD_ROWS)
    wq_first = [[remote(wq_all.at[0, d, pl.ds(o, n)], wq_all.at[1 + d, d, pl.ds(o, n)], d)
                 for o, n in WQ_CHUNKS] for d in range(2)]
    wq_second = [remote(wq_all.at[0, 1 - d, rest], wq_all.at[1 + d, 1 - d, rest], d)
                 for d in range(2)]
    link_open = (me >= 2, jnp.logical_or(me == 1, me == 2))

    def load_kv(s, q):
        src = (pl.ds(2 * me, 2), slot_group[s] * 2 + q)
        return load(kt_hbm.at[src], kt_f.at[s, q]), load(vt_hbm.at[src], vt_f.at[s, q])

    kv_ld = {}
    for ci, (o, n) in enumerate(WQ_CHUNKS):
        wq_ld[ci].wait()
        for q in range(2):
            wq_all[0, q, o:o + n, :] = wq_f[o:o + n, q * 128:(q + 1) * 128].astype(BF)
        for d in range(2):
            @pl.when(link_open[d])
            def _():
                wq_first[d][ci].start()
                if ci == len(WQ_CHUNKS) - 1:
                    wq_second[d].start()
        if ci == 0:
            x_ld = load(x_hbm, x_f)
            kv_ld[(0, 0)] = load_kv(0, 0)
            wo_ld = load(wo_hbm, wo_f)
            for sq in ((0, 1), (1, 0), (2, 1), (1, 1), (2, 0), (3, 0), (3, 1)):
                kv_ld[sq] = load_kv(*sq)

    def late_start(d):
        for cp in wq_first[d] + [head[d], wq_second[d]]:
            cp.start()

    @pl.when(me == 0)
    def _():
        pl.semaphore_wait(bar, 2)
        late_start(0)
        late_start(1)

    for pos, d in ((1, 0), (3, 1)):
        @pl.when(me == pos)
        def _():
            pl.semaphore_wait(rdy, 1)
            late_start(d)

    x_ld.wait()
    x_b[...] = x_f[...].astype(BF)

    lo = lax.broadcasted_iota(jnp.int32, (64, 128), 1) < 64
    on_diag = ((lax.broadcasted_iota(jnp.int32, (128, 128), 0) < 64)
               == (lax.broadcasted_iota(jnp.int32, (128, 128), 1) < 64))
    neg = jnp.float32(-jnp.inf)

    def softmax_halves(s):
        m_lo = jnp.max(jnp.where(lo, s, neg), axis=-1, keepdims=True)
        m_hi = jnp.max(jnp.where(lo, neg, s), axis=-1, keepdims=True)
        p = jnp.exp(s - jnp.where(lo, m_lo, m_hi))
        l_lo = jnp.sum(jnp.where(lo, p, 0.0), axis=-1, keepdims=True)
        l_hi = jnp.sum(jnp.where(lo, 0.0, p), axis=-1, keepdims=True)
        return (p * jnp.where(lo, 1.0 / l_lo, 1.0 / l_hi)).astype(BF)

    def attend(s, q, kv_wait_first=True):
        def wait_kv():
            for cp in kv_ld[(s, q)]:
                cp.wait()

        if kv_wait_first:
            wait_kv()
        qp = jnp.dot(x_b[...], wq_all[s, q], preferred_element_type=F32) * 0.125
        if not kv_wait_first:
            wait_kv()
        nt = (((1,), (1,)), ((), ()))
        for b in range(2):
            for g in range(2):
                r0 = b * 256 + g * 128
                qa = qp[r0:r0 + 64]
                qb = qp[r0 + 64:r0 + 128]
                kk = kt_f[s, q, b, :, g * 128:(g + 1) * 128]
                vv = vt_f[s, q, b, :, g * 128:(g + 1) * 128]
                s1 = jnp.dot(jnp.where(lo, qa, qb).astype(BF),
                             jnp.where(on_diag, kk, 0.0).astype(BF),
                             preferred_element_type=F32)
                s2 = jnp.dot(jnp.where(lo, qb, qa).astype(BF),
                             jnp.where(on_diag, 0.0, kk).astype(BF),
                             preferred_element_type=F32)
                c1 = lax.dot_general(softmax_halves(s1),
                                     jnp.where(on_diag, vv, 0.0).astype(BF),
                                     nt, preferred_element_type=F32)
                c2 = lax.dot_general(softmax_halves(s2),
                                     jnp.where(on_diag, 0.0, vv).astype(BF),
                                     nt, preferred_element_type=F32)
                ctx[s, q, r0:r0 + 64, :] = jnp.where(lo, c1, c2).astype(BF)
                ctx[s, q, r0 + 64:r0 + 128, :] = jnp.where(lo, c2, c1).astype(BF)

    def wo_tile(s, q, n):
        if n < 3:
            return wo_all[s, q, n * 128:(n + 1) * 128, :]
        r = 384 + 64 * q
        return jnp.concatenate([wo_all[s, 0, r:r + 64, :], wo_all[s, 1, r:r + 64, :]], axis=0)

    def project(terms, n, first=False, last=False, split=1):
        rows = T // split
        tiles = [wo_tile(s, q, n) for s, q in terms]
        for i in range(split):
            rs = slice(i * rows, (i + 1) * rows)
            r = None if first else acc[n, rs, :]
            for (s, q), w in zip(terms, tiles):
                t = jnp.dot(ctx[s, q, rs, :], w, preferred_element_type=F32)
                r = t if r is None else r + t
            if last:
                out_ref[rs, n * 128:(n + 1) * 128] = r
            else:
                acc[n, rs, :] = r

    def wait_recv(cps):
        for cp in cps:
            cp.wait_recv()

    def send_wo(src_slot, dst_slot, stream, rows):
        return [send(wo_all.at[src_slot(d), stream(d), rows],
                     wo_all.at[dst_slot(d), stream(d), rows], d) for d in range(2)]

    def send_own_wo(stream, rows):
        return send_wo(lambda d: 0, lambda d: 1 + d, stream, rows)

    def forward_wo(o, n):
        return send_wo(lambda d: 1 + d, lambda d: 3, lambda d: d, pl.ds(o, n))

    attend(0, 0, kv_wait_first=False)
    wo_ld.wait()
    for q in range(2):
        for n in range(3):
            wo_all[0, q, n * 128:(n + 1) * 128, :] = (
                wo_f[q * 128:(q + 1) * 128, n * 128:(n + 1) * 128].astype(BF))
        for d in range(2):
            r = q * 128 + d * 64
            wo_all[0, d, 384 + 64 * q:448 + 64 * q, :] = wo_f[r:r + 64, 384:512].astype(BF)
    wo_first_a = send_own_wo(lambda d: d, pl.ds(0, 256))
    attend(0, 1, kv_wait_first=False)

    wait_recv(wq_first[0] + wq_first[1])
    wq_fwd = [send(wq_all.at[1 + d, d], wq_all.at[3, d], d) for d in range(2)]
    wo_first_b = send_own_wo(lambda d: d, pl.ds(256, 256))
    n_done_early = len(sends)
    wo_second = send_own_wo(lambda d: 1 - d, pl.ds(0, 512))
    attend(1, 0)
    attend(2, 1)

    wait_recv(head + wq_second)
    for d in range(2):
        wq_all[1 + d, 1 - d, 0:HEAD_ROWS, :] = head_buf[d].astype(BF)
    attend(1, 1)
    attend(2, 0)

    wait_recv(wo_first_a)
    wo_fwd = [forward_wo(o, n) for o, n in FWD_WO[:2]]
    for n in range(2):
        project(((0, 0), (0, 1), (1, 0), (2, 1)), n, first=True)
    for n in range(2, 4):
        project(((0, 0), (0, 1)), n, first=True)

    wait_recv(wq_fwd)
    attend(3, 0)
    attend(3, 1)

    wait_recv(wo_first_b)
    wo_fwd += [forward_wo(o, n) for o, n in FWD_WO[2:]]
    project(((1, 0), (2, 1)), 2, split=2)
    for cp in sends[:n_done_early]:
        cp.wait_send()

    wait_recv(wo_second)
    for n in range(3):
        project(((1, 1), (2, 0)), n)
    project(((1, 0), (1, 1), (2, 0), (2, 1)), 3)

    for n in range(3):
        wait_recv(wo_fwd[n])
        project(((3, 0), (3, 1)), n, last=True, split=2)
    wait_recv(wo_fwd[3])
    project(((3, 0),), 3, split=4)
    for cp in sends[n_done_early:]:
        cp.wait_send()
    wait_recv(wo_fwd[4])
    project(((3, 1),), 3, last=True, split=4)

    assert counts["local"] == N_LOCAL and counts["remote"] == N_REMOTE


def _kernel(*refs):
    pl.run_scoped(
        lambda *sems: _body(*refs, *sems),
        pltpu.SemaphoreType.DMA((N_LOCAL,)),
        pltpu.SemaphoreType.DMA((N_REMOTE,)),
        pltpu.SemaphoreType.DMA((N_REMOTE,)),
        pltpu.SemaphoreType.REGULAR,
    )


def pallas_dist_sparse_attn_strided_htp_bs_b2_sq256_skv256_hq4_dh64_kernel(
    x: jax.Array,
    Wq: jax.Array,
    K_ext: jax.Array,
    V_ext: jax.Array,
    Wo: jax.Array,
):
    kt = jnp.transpose(K_ext, (0, 2, 3, 1)).reshape(8, 8, 128, 256)
    vt = jnp.transpose(V_ext, (0, 2, 3, 1)).reshape(8, 8, 128, 256)

    out = pl.pallas_call(
        _kernel,
        out_shape=jax.ShapeDtypeStruct((T, D), F32),
        in_specs=[pl.BlockSpec(memory_space=pl.ANY)] * 5,
        out_specs=pl.BlockSpec(memory_space=pltpu.VMEM),
        scratch_shapes=[
            pltpu.VMEM((T, D), F32),
            pltpu.VMEM((512, 256), F32),
            pltpu.VMEM((256, 512), F32),
            pltpu.VMEM((4, 2, 2, 128, 256), F32),
            pltpu.VMEM((4, 2, 2, 128, 256), F32),
            pltpu.VMEM((T, D), BF),
            pltpu.VMEM((4, 2, 512, 128), BF),
            pltpu.VMEM((4, 2, 512, 128), BF),
            pltpu.VMEM((4, 2, T, 128), BF),
            pltpu.VMEM((4, T, 128), F32),
            pltpu.VMEM((2, HEAD_ROWS, 128), F32),
        ],
        compiler_params=pltpu.CompilerParams(
            collective_id=0, vmem_limit_bytes=64 * 1024 * 1024),
    )(x.reshape(T, D), Wq, kt, vt, Wo)
    return out.reshape(2, 256, D)
```
